```python
import numpy as np

kernel_name = "dist_matmul_relu_kshard_i_m1024_n1024_k512"

def setup_inputs():
    A = np.random.randn(1024, 2048).astype(np.float32)
    B = np.random.randn(2048, 1024).astype(np.float32)
    return {"A": A, "B": B}

def reference(A: np.ndarray, B: np.ndarray) -> np.ndarray:
    z = A @ B
    return np.maximum(z, 0.0)
```

```python
import contextlib
import jax
import jax.numpy as jnp
from jax import lax
from jax.experimental import pallas as pl
from jax.experimental.pallas import tpu as pltpu

M, N, KS = 1024, 1024, 512
H = M // 2
BF = jnp.bfloat16
F32 = jnp.float32


def make_kernel(R=232, arows=(48, 48, 32), bcols=(128,) * 8,
                order="b0 a0 a1 b1 a2 b2 b3 b4 b5 b6 b7 a3 e k", ahead=3,
                s1="0:1,0:1 1:2,0:1 0:2,1:2 2:3,0:2 0:3,2:3 0:3,3:4 0:3,4:5 0:3,5:6 0:3,6:7 0:3,7:8 3:4,0:8",
                s2=(128,), s3=(128,), cp=dict(disable_semaphore_checks=True), scopes=False, Er=40):
    E = H - 2 * R
    Er = E if Er is None else Er
    Ed = E - Er

    def ranges(ch, tot):
        ch = tuple(ch) + ((tot - sum(ch),) if sum(ch) < tot else ())
        out, j = [], 0
        for c in ch:
            out.append((j, j + c)); j += c
        return out
    ar, bc, r2, r3 = ranges(arows, R), ranges(bcols, N), ranges(s2, R), ranges(s3, R)
    s1 = [tuple(tuple(int(v) for v in t.split(":")) for t in m.split(",")) for m in s1.split()]
    m1 = [(ar[a0][0], ar[a1 - 1][1], bc[b0][0], bc[b1 - 1][1]) for (a0, a1), (b0, b1) in s1]
    assert sum((r1 - r0) * (c1 - c0) for r0, r1, c0, c1 in m1) == R * N
    order = [o for o in order.split() if E or o != "e"]
    n1, n2, n3 = len(m1), len(r2), len(r3)
    scope = (lambda n: jax.named_scope(n)) if scopes else (lambda n: contextlib.nullcontext())
    al = 16 if R % 16 == 0 else 8

    def body(a_hbm, b_hbm, o_ref, a32, b32, s2s, s2r, ez, e1s, e1r, e2s, e2r, *rest):
        s1s, s1r = rest[:n1], rest[n1:2 * n1]
        lsem, ss1, rs1, ss2, rs2, ss3, rs3, sse, rse = rest[2 * n1:]
        p = lax.axis_index("i")
        x = p >> 1
        y = (p ^ x) & 1
        co = (x, y)
        nbr = (p ^ 3, p ^ 1)
        row = (R * (1 - x), H + R * (1 - y), R * x, H + R * y)
        row = [pl.multiple_of(r, al) for r in row]

        loads = {}
        k = 0
        for i, (r0, r1) in enumerate(ar):
            loads[f"a{i}"] = [pltpu.make_async_copy(a_hbm.at[pl.ds(row[h] + r0, r1 - r0), :],
                                                    a32.at[pl.ds(2 * r0 + h * (r1 - r0), r1 - r0), :], lsem.at[k + h]) for h in range(2)]
            k += 2
        for j, (c0, c1) in enumerate(bc):
            loads[f"b{j}"] = [pltpu.make_async_copy(b_hbm.at[:, pl.ds(c0, c1 - c0)], b32.at[:, pl.ds(c0, c1 - c0)], lsem.at[k])]
            k += 1
        if E:
            loads["e"] = [pltpu.make_async_copy(a_hbm.at[pl.ds(h * H + 2 * R, E), :], a32.at[pl.ds(2 * R + h * E, E), :], lsem.at[k + h]) for h in range(2)]
        k += 2
        K0 = 2 * R + 2 * E
        loads["k"] = [pltpu.make_async_copy(a_hbm.at[pl.ds(row[2 + h], R), :], a32.at[pl.ds(K0 + h * R, R), :], lsem.at[k + h]) for h in range(2)]
        started, done = [0], set()

        def start_until(n):
            while started[0] < min(n, len(order)):
                for c_ in loads[order[started[0]]]:
                    c_.start()
                started[0] += 1

        def wait_load(nm):
            if nm in done:
                return
            start_until(order.index(nm) + 1)
            with scope(f"wl_{nm}"):
                for c_ in loads[nm]:
                    c_.wait()
            done.add(nm)
            start_until(len(done) + ahead)

        start_until(ahead)
        bar = pltpu.get_barrier_semaphore()
        for l in range(2):
            pl.semaphore_signal(bar, inc=1, device_id=(nbr[l],), device_id_type=pl.DeviceIdType.MESH)

        def rc(src, dst, ssem, rsem, link):
            return pltpu.make_async_remote_copy(src_ref=src, dst_ref=dst, send_sem=ssem, recv_sem=rsem,
                                                device_id=(nbr[link],), device_id_type=pl.DeviceIdType.MESH)

        c1 = [[rc(s1s[c].at[h], s1r[c].at[h], ss1.at[h * n1 + c], rs1.at[h * n1 + c], h) for c in range(n1)] for h in range(2)]
        c2 = [[rc(s2s.at[h, pl.ds(r0, r1 - r0)], s2r.at[h, pl.ds(r0, r1 - r0)], ss2.at[h * n2 + c], rs2.at[h * n2 + c], 1 - h)
               for c, (r0, r1) in enumerate(r2)] for h in range(2)]
        c3 = [[rc(o_ref.at[pl.ds(row[2 + h] + r0, r1 - r0)], o_ref.at[pl.ds(row[2 + h] + r0, r1 - r0)],
                  ss3.at[h * n3 + c], rs3.at[h * n3 + c], h) for c, (r0, r1) in enumerate(r3)] for h in range(2)]
        c3r = [[rc(o_ref.at[pl.ds(row[h] + r0, r1 - r0)], o_ref.at[pl.ds(row[h] + r0, r1 - r0)],
                   ss3.at[h * n3 + c], rs3.at[h * n3 + c], h) for c, (r0, r1) in enumerate(r3)] for h in range(2)]
        if E:
            oe = [o_ref.at[pl.ds(h * H + 2 * R, E)] for h in range(2)]
            ce1 = [rc(e1s.at[h], e1r.at[h], sse.at[h], rse.at[h], h) for h in range(2)]
            ce2 = [rc(e2s.at[h], e2r.at[h], sse.at[2 + h], rse.at[2 + h], 1 - h) for h in range(2)]
            ce3 = [rc(oe[h], oe[h], sse.at[4 + h], rse.at[4 + h], h) for h in range(2)]
            oer = [o_ref.at[pl.ds(h * H + 2 * R + Ed, Er)] for h in range(2)]
            ce4 = [rc(oer[h], oer[h], sse.at[6 + h], rse.at[6 + h], 1 - h) for h in range(2)]
            if Ed:
                oed = [o_ref.at[pl.ds(h * H + 2 * R, Ed)] for h in range(2)]
                ce5 = [rc(oed[h], oed[h], sse.at[8 + h], rse.at[8 + h], h) for h in range(2)]

        for c, ((a0, a1), (b0, b1)) in enumerate(s1):
            r0, r1, q0, q1 = m1[c]
            units, j = [], b0
            while j < b1:
                e = j + 1
                if f"b{j}" in done:
                    while e < b1 and f"b{e}" in done:
                        e += 1
                units.append((j, e)); j = e
            for ui, (j0, j1) in enumerate(units):
                u0, u1 = bc[j0][0], bc[j1 - 1][1]
                for nm in order:
                    if nm == f"b{j0}" or (nm[0] == "a" and a0 <= int(nm[1:]) < a1):
                        wait_load(nm)
                z = jnp.dot(a32[2 * r0:2 * r1, :], b32[:, u0:u1], preferred_element_type=F32).astype(BF)
                for i in range(a0, a1):
                    w0, w1 = ar[i]
                    for h in range(2):
                        o = 2 * (w0 - r0) + h * (w1 - w0)
                        s1s[c][h, w0 - r0:w1 - r0, u0 - q0:u1 - q0] = z[o:o + w1 - w0]
            if c == 0:
                with scope("bar"):
                    pl.semaphore_wait(bar, 2)
            with scope(f"s1_{c}"):
                for h in range(2):
                    c1[h][c].start()
        if E:
            wait_load("e")
            z = jnp.dot(a32[2 * R:2 * R + 2 * E, :], b32[...], preferred_element_type=F32)
            ez[...] = z
            for h in range(2):
                @pl.when(co[h] == 0)
                def _():
                    e1s[h] = z[h * E:(h + 1) * E].astype(BF)
                    ce1[h].start()
        wait_load("k")

        got = set()
        for c, (r0, r1) in enumerate(r2):
            for h in range(2):
                z = jnp.dot(a32[K0 + h * R + r0:K0 + h * R + r1, :], b32[...], preferred_element_type=F32)
                for d, (u0, u1, q0, q1) in enumerate(m1):
                    lo, hi = max(r0, u0), min(r1, u1)
                    if lo >= hi:
                        continue
                    if (h, d) not in got:
                        with scope(f"r1_{d}_{h}"):
                            c1[h][d].wait_recv()
                        got.add((h, d))
                    s2s[h, lo:hi, q0:q1] = (z[lo - r0:hi - r0, q0:q1] + s1r[d][h, lo - u0:hi - u0, :].astype(F32)).astype(BF)
                if E and c == n2 - 1:
                    @pl.when(co[h] == 1)
                    def _():
                        with scope(f"re1_{h}"):
                            ce1[h].wait_recv()
                        e2s[h] = (ez[h * E:(h + 1) * E] + e1r[h].astype(F32)).astype(BF)
                        ce2[h].start()
                with scope(f"s2_{c}_{h}"):
                    c2[h][c].start()

        got = set()
        for c, (r0, r1) in enumerate(r3):
            for h in range(2):
                if E and c == 0:
                    @pl.when(co[h] == 1)
                    def _():
                        with scope(f"re2_{h}"):
                            ce2[h].wait_recv()
                        oe[h][...] = jnp.maximum(e2s[h].astype(F32) + e2r[h].astype(F32), 0.0).astype(BF)

                        @pl.when(co[1 - h] == 0)
                        def _():
                            ce3[h].start()
                        if Ed:
                            @pl.when(co[1 - h] == 1)
                            def _():
                                ce5[h].start()
                for d, (u0, u1) in enumerate(r2):
                    if max(r0, u0) < min(r1, u1) and (h, d) not in got:
                        with scope(f"r2_{d}_{h}"):
                            c2[h][d].wait_recv()
                        got.add((h, d))
                f = jnp.maximum(s2s[h, r0:r1, :].astype(F32) + s2r[h, r0:r1, :].astype(F32), 0.0).astype(BF)
                o_ref[pl.ds(row[2 + h] + r0, r1 - r0), :] = f
                with scope(f"s3_{c}_{h}"):
                    c3[h][c].start()

        if E:
            @pl.when(p == 0)
            def _():
                for h in range(2):
                    with scope(f"re3_{h}"):
                        ce3[h].wait_recv()
                    ce4[h].start()
                for h in range(2):
                    ce4[h].wait_send()
            for h in range(2):
                @pl.when(co[h] == 0)
                def _():
                    ce1[h].wait_send()

                    @pl.when(co[1 - h] == 1)
                    def _():
                        with scope(f"re4_{h}"):
                            ce4[h].wait_recv()
                        if Ed:
                            ce5[h].wait_recv()

                @pl.when(co[h] == 1)
                def _():
                    ce2[h].wait_send()

                    @pl.when(co[1 - h] == 0)
                    def _():
                        ce3[h].wait_send()
                    if Ed:
                        @pl.when(co[1 - h] == 1)
                        def _():
                            ce5[h].wait_send()

        for cs in (c1, c2, c3):
            for h in range(2):
                for c_ in cs[h]:
                    c_.wait_send()
        for h in range(2):
            for d, c_ in enumerate(c3r[h]):
                with scope(f"r3_{d}_{h}"):
                    c_.wait_recv()

    Ea = max(E, 16)

    def fn(A, B):
        return pl.pallas_call(
            body,
            out_shape=pltpu.VMEM((M, N), BF),
            in_specs=[pl.BlockSpec(memory_space=pltpu.HBM), pl.BlockSpec(memory_space=pltpu.HBM)],
            out_specs=pl.BlockSpec(memory_space=pltpu.VMEM),
            scratch_shapes=[
                pltpu.VMEM((M, KS), F32), pltpu.VMEM((KS, N), F32),
                pltpu.VMEM((2, R, N), BF), pltpu.VMEM((2, R, N), BF),
                pltpu.VMEM((2 * Ea, N), F32), *[pltpu.VMEM((2, Ea, N), BF) for _ in range(4)],
                *[pltpu.VMEM((2, r1 - r0, q1 - q0), BF) for r0, r1, q0, q1 in m1],
                *[pltpu.VMEM((2, r1 - r0, q1 - q0), BF) for r0, r1, q0, q1 in m1],
                pltpu.SemaphoreType.DMA((2 * len(ar) + len(bc) + 4,)),
                pltpu.SemaphoreType.DMA((2 * n1,)), pltpu.SemaphoreType.DMA((2 * n1,)),
                pltpu.SemaphoreType.DMA((2 * n2,)), pltpu.SemaphoreType.DMA((2 * n2,)),
                pltpu.SemaphoreType.DMA((2 * n3,)), pltpu.SemaphoreType.DMA((2 * n3,)),
                pltpu.SemaphoreType.DMA((10,)), pltpu.SemaphoreType.DMA((10,)),
            ],
            compiler_params=pltpu.CompilerParams(collective_id=0, vmem_limit_bytes=64 << 20, **cp),
        )(A, B)
    return fn


def pallas_dist_matmul_relu_kshard_i_m1024_n1024_k512_kernel(A, B):
    return make_kernel()(A, B)
```

```python
import jax
import jax.numpy as jnp
from jax import lax
from jax.experimental import pallas as pl
from jax.experimental.pallas import tpu as pltpu

M, N, KS = 1024, 1024, 512
HALF = M // 2
OUTER = 128
MID = HALF - 2 * OUTER
LANES = 128
BF16, F32 = jnp.bfloat16, jnp.float32

A_PIECES = ((0, 80), (80, OUTER))
B_BLOCKS = tuple((q, q + LANES) for q in range(0, N, LANES))
FIRST_MESSAGES = (((0, 1), (0, 1)), ((0, 1), (1, 2)), ((1, 2), (0, 2))) + tuple(
    ((0, 2), (j, j + 1)) for j in range(2, len(B_BLOCKS))
)
GROUPS = ((0, 384, 96, 32), (384, N, 112, 32))

PARTIAL, PAIR_SUM, TO_RELAY, FINISHED, RELAYED = range(5)


def _extent(message):
    (a0, a1), (b0, b1) = message
    return A_PIECES[a0][0], A_PIECES[a1 - 1][1], B_BLOCKS[b0][0], B_BLOCKS[b1 - 1][1]


def _owned(g, c):
    return (0, GROUPS[g][2]) if c == 0 else (GROUPS[g][2], MID)


def _via_relay(g):
    return GROUPS[g][2], GROUPS[g][2] + GROUPS[g][3]


def _direct(g, c):
    return _owned(g, 0) if c == 0 else (_via_relay(g)[1], MID)


def _matmul(a, b):
    return jnp.dot(a.astype(BF16), b.astype(BF16), preferred_element_type=F32)


def _finish(mine, theirs):
    return jnp.maximum(mine.astype(F32) + theirs.astype(F32), 0.0).astype(BF16)


def _body(a_hbm, b_hbm, out_ref, a_buf, b_buf, mid_partial, mid1_send, mid1_recv,
          mid2_send, mid2_recv, out2_send, out2_recv, load_sems, first_send_sems,
          first_recv_sems, outer_send_sems, outer_recv_sems, mid_send_sems,
          mid_recv_sems, *first_bufs):
    n_first, n_groups = len(FIRST_MESSAGES), len(GROUPS)
    out1_send, out1_recv = first_bufs[:n_first], first_bufs[n_first:]
    halves, groups = range(2), range(n_groups)

    me = lax.axis_index("i")
    x = me >> 1
    coord = (x, (me ^ x) & 1)
    neighbour = (me ^ 3, me ^ 1)
    send_row = [pl.multiple_of(h * HALF + (HALF - OUTER) * (1 - coord[h]), OUTER) for h in halves]
    keep_row = [pl.multiple_of(h * HALF + (HALF - OUTER) * coord[h], OUTER) for h in halves]

    mid_at, keep_at = 2 * OUTER, 2 * OUTER + 2 * MID
    sem_ids = iter(range(2 * len(A_PIECES) + len(B_BLOCKS) + 4))

    def load_a(hbm_row, buf_row, rows):
        return pltpu.make_async_copy(
            a_hbm.at[pl.ds(hbm_row, rows)], a_buf.at[pl.ds(buf_row, rows)],
            load_sems.at[next(sem_ids)])

    load_piece = [
        [load_a(send_row[h] + r0, 2 * r0 + h * (r1 - r0), r1 - r0) for h in halves]
        for r0, r1 in A_PIECES
    ]
    load_block = [
        [pltpu.make_async_copy(
            b_hbm.at[:, pl.ds(q0, q1 - q0)], b_buf.at[:, pl.ds(q0, q1 - q0)],
            load_sems.at[next(sem_ids)])]
        for q0, q1 in B_BLOCKS
    ]
    load_mid = [load_a(h * HALF + OUTER, mid_at + h * MID, MID) for h in halves]
    load_keep = [load_a(keep_row[h], keep_at + h * OUTER, OUTER) for h in halves]

    pending = [load_block[0], load_piece[0], load_block[1], load_piece[1], *load_block[2:]]
    for copies in pending[:2]:
        for copy in copies:
            copy.start()
    barrier = pltpu.get_barrier_semaphore()
    for link in range(2):
        pl.semaphore_signal(barrier, inc=1, device_id=(neighbour[link],),
                            device_id_type=pl.DeviceIdType.MESH)
    for copies in (*pending[2:], load_mid, load_keep):
        for copy in copies:
            copy.start()

    def await_loads(needed):
        for copies in list(pending):
            if any(copies is n for n in needed):
                for copy in copies:
                    copy.wait()
                pending[:] = [p for p in pending if p is not copies]

    def remote(src, dst, send_sem, recv_sem, link):
        return pltpu.make_async_remote_copy(
            src_ref=src, dst_ref=dst, send_sem=send_sem, recv_sem=recv_sem,
            device_id=(neighbour[link],), device_id_type=pl.DeviceIdType.MESH)

    def outer_partial(h, m):
        s = h * n_first + m
        return remote(out1_send[m].at[h], out1_recv[m].at[h],
                      first_send_sems.at[s], first_recv_sems.at[s], h)

    def outer_pair_sum(h):
        return remote(out2_send.at[h], out2_recv.at[h],
                      outer_send_sems.at[h], outer_recv_sems.at[h], 1 - h)

    def outer_finished(h, row):
        rows = out_ref.at[pl.ds(row, OUTER)]
        return remote(rows, rows, outer_send_sems.at[2 + h], outer_recv_sems.at[2 + h], h)

    def middle(kind, h, g, rows):
        r0, r1 = rows
        cols = pl.ds(GROUPS[g][0], GROUPS[g][1] - GROUPS[g][0])
        if kind == PARTIAL:
            src, dst = (b.at[h, pl.ds(r0, r1 - r0), cols] for b in (mid1_send, mid1_recv))
        elif kind == PAIR_SUM:
            src, dst = (b.at[h, pl.ds(r0, r1 - r0), cols] for b in (mid2_send, mid2_recv))
        else:
            src = dst = out_ref.at[pl.ds(h * HALF + OUTER + r0, r1 - r0), cols]
        s = (kind * 2 + h) * n_groups + g
        link = 1 - h if kind in (PAIR_SUM, RELAYED) else h
        return remote(src, dst, mid_send_sems.at[s], mid_recv_sems.at[s], link)

    def by_coordinate(h, fn):
        for c in range(2):
            pl.when(coord[h] == c)(lambda c=c: fn(h, c))

    for m, message in enumerate(FIRST_MESSAGES):
        (a0, a1), (b0, b1) = message
        r0, r1, q0, q1 = _extent(message)
        await_loads(load_piece[a0:a1] + load_block[b0:b1])
        z = _matmul(a_buf[2 * r0:2 * r1, :], b_buf[:, q0:q1]).astype(BF16)
        for p0, p1 in A_PIECES[a0:a1]:
            for h in halves:
                at = 2 * (p0 - r0) + h * (p1 - p0)
                out1_send[m][h, p0 - r0:p1 - r0, :] = z[at:at + p1 - p0]
        if m == 0:
            pl.semaphore_wait(barrier, 2)
        for h in halves:
            outer_partial(h, m).start()

    for g in groups:
        q0, q1 = GROUPS[g][:2]
        for h in halves:
            if g == 0:
                load_mid[h].wait()
            z = _matmul(a_buf[mid_at + h * MID:mid_at + (h + 1) * MID, :], b_buf[:, q0:q1])
            mid_partial[h, :, q0:q1] = z
            mid1_send[h, :, q0:q1] = z.astype(BF16)
            by_coordinate(h, lambda h, c: middle(PARTIAL, h, g, _owned(g, 1 - c)).start())

    for h in halves:
        load_keep[h].wait()
        z = _matmul(a_buf[keep_at + h * OUTER:keep_at + (h + 1) * OUTER, :], b_buf[...])
        for m, message in enumerate(FIRST_MESSAGES):
            r0, r1, q0, q1 = _extent(message)
            outer_partial(h, m).wait_recv()
            out2_send[h, r0:r1, q0:q1] = (
                z[r0:r1, q0:q1] + out1_recv[m][h].astype(F32)).astype(BF16)
        outer_pair_sum(h).start()

    def middle_pair_sums(h, c):
        for g in groups:
            (r0, r1), (q0, q1) = _owned(g, c), GROUPS[g][:2]
            middle(PARTIAL, h, g, (r0, r1)).wait_recv()
            mid2_send[h, r0:r1, q0:q1] = (
                mid_partial[h, r0:r1, q0:q1] + mid1_recv[h, r0:r1, q0:q1].astype(F32)
            ).astype(BF16)
            middle(PAIR_SUM, h, g, (r0, r1)).start()

    for h in halves:
        by_coordinate(h, middle_pair_sums)

    for h in halves:
        outer_pair_sum(h).wait_recv()
        out_ref[pl.ds(keep_row[h], OUTER), :] = _finish(out2_send[h], out2_recv[h])
        outer_finished(h, keep_row[h]).start()

    def middle_finished(h, c):
        top = h * HALF + OUTER
        for g in groups:
            (r0, r1), (q0, q1) = _owned(g, c), GROUPS[g][:2]
            middle(PAIR_SUM, h, g, (r0, r1)).wait_recv()
            out_ref[top + r0:top + r1, q0:q1] = _finish(
                mid2_send[h, r0:r1, q0:q1], mid2_recv[h, r0:r1, q0:q1])
        if c == 1:
            @pl.when(coord[1 - h] == 0)
            def _():
                for g in groups:
                    middle(TO_RELAY, h, g, _via_relay(g)).start()
        for g in groups:
            middle(FINISHED, h, g, _direct(g, c)).start()

    for h in halves:
        by_coordinate(h, middle_finished)

    @pl.when(me == 0)
    def _():
        for h in halves:
            for g in groups:
                middle(TO_RELAY, h, g, _via_relay(g)).wait_recv()
                middle(RELAYED, h, g, _via_relay(g)).start()
        for h in halves:
            for g in groups:
                middle(RELAYED, h, g, _via_relay(g)).wait_send()

    def drain_middle(h, c):
        for g in groups:
            middle(PARTIAL, h, g, _owned(g, 1 - c)).wait_send()
            middle(PAIR_SUM, h, g, _owned(g, c)).wait_send()
            middle(FINISHED, h, g, _direct(g, c)).wait_send()
            middle(FINISHED, h, g, _direct(g, 1 - c)).wait_recv()
        if c == 1:
            @pl.when(coord[1 - h] == 0)
            def _():
                for g in groups:
                    middle(TO_RELAY, h, g, _via_relay(g)).wait_send()
        else:
            @pl.when(coord[1 - h] == 1)
            def _():
                for g in groups:
                    middle(RELAYED, h, g, _via_relay(g)).wait_recv()

    for h in halves:
        for m in range(n_first):
            outer_partial(h, m).wait_send()
        outer_pair_sum(h).wait_send()
        outer_finished(h, keep_row[h]).wait_send()
        outer_finished(h, send_row[h]).wait_recv()
        by_coordinate(h, drain_middle)


def pallas_dist_matmul_relu_kshard_i_m1024_n1024_k512_kernel(
    A: jax.Array,
    B: jax.Array,
):
    assert A.shape == (M, KS) and B.shape == (KS, N), (A.shape, B.shape)
    first_bufs = [
        pltpu.VMEM((2, r1 - r0, q1 - q0), BF16)
        for r0, r1, q0, q1 in map(_extent, FIRST_MESSAGES)
    ]
    dma = pltpu.SemaphoreType.DMA
    return pl.pallas_call(
        _body,
        out_shape=pltpu.VMEM((M, N), BF16),
        in_specs=[pl.BlockSpec(memory_space=pltpu.HBM)] * 2,
        out_specs=pl.BlockSpec(memory_space=pltpu.VMEM),
        scratch_shapes=[
            pltpu.VMEM((M, KS), A.dtype),
            pltpu.VMEM((KS, N), B.dtype),
            pltpu.VMEM((2, MID, N), F32),
            pltpu.VMEM((2, MID, N), BF16),
            pltpu.VMEM((2, MID, N), BF16),
            pltpu.VMEM((2, MID, N), BF16),
            pltpu.VMEM((2, MID, N), BF16),
            pltpu.VMEM((2, OUTER, N), BF16),
            pltpu.VMEM((2, OUTER, N), BF16),
            dma((2 * len(A_PIECES) + len(B_BLOCKS) + 4,)),
            dma((2 * len(FIRST_MESSAGES),)),
            dma((2 * len(FIRST_MESSAGES),)),
            dma((4,)),
            dma((4,)),
            dma((10 * len(GROUPS),)),
            dma((10 * len(GROUPS),)),
            *first_bufs,
            *first_bufs,
        ],
        compiler_params=pltpu.CompilerParams(
            collective_id=0,
            vmem_limit_bytes=64 * 1024 * 1024,
            disable_semaphore_checks=True,
        ),
    )(A, B)
```
